```python
import numpy as np

kernel_name = "dist_rope_attn_htp_bs_b2_sq512_d1024_hq8_dh128"

def setup_inputs():
    x = np.random.randn(8, 512, 1024).astype(np.float32)
    Wq = np.random.randn(1024, 4096).astype(np.float32) * 0.02
    Wk = np.random.randn(1024, 4096).astype(np.float32) * 0.02
    Wv = np.random.randn(1024, 4096).astype(np.float32) * 0.02
    Wo = np.random.randn(4096, 1024).astype(np.float32) * 0.02
    return {"x": x, "Wq": Wq, "Wk": Wk, "Wv": Wv, "Wo": Wo}

def reference(x, Wq, Wk, Wv, Wo):
    B, Sq, Hq, Dh = 8, 512, 32, 128
    inv = 1.0 / (10000.0 ** (np.arange(0, Dh, 2) / Dh))
    pos = np.arange(Sq)[:, None] * inv[None, :]
    cos = np.repeat(np.cos(pos), 2, axis=-1).astype(np.float32)
    sin = np.repeat(np.sin(pos), 2, axis=-1).astype(np.float32)
    def rot(t):
        t2 = t.reshape(B, Sq, Hq, Dh // 2, 2)
        t_r = np.stack([-t2[..., 1], t2[..., 0]], axis=-1).reshape(B, Sq, Hq, Dh)
        return t * cos[None, :, None, :] + t_r * sin[None, :, None, :]
    Q = rot((x @ Wq).reshape(B, Sq, Hq, Dh))
    K = rot((x @ Wk).reshape(B, Sq, Hq, Dh))
    V = (x @ Wv).reshape(B, Sq, Hq, Dh)
    s = np.einsum('bihd,bjhd->bhij', Q, K).astype(np.float32) * 0.08838834764831843
    s_max = s.max(axis=-1, keepdims=True)
    w = np.exp(s - s_max)
    w = w / w.sum(axis=-1, keepdims=True)
    ctx = np.einsum('bhij,bjhd->bihd', w, V).reshape(B, Sq, Hq * Dh)
    return ctx @ Wo
```

```python
import jax
import jax.numpy as jnp
from jax import lax
from jax.experimental import pallas as pl
from jax.experimental.pallas import tpu as pltpu

N_DEV = 4
B_LOC = 2
SQ = 512
D = 1024
HQ = 8
DH = 128
SCALE = 0.08838834764831843
CH = 256

F32 = jnp.float32
BF16 = jnp.bfloat16


def pallas_dist_rope_attn_htp_bs_b2_sq512_d1024_hq8_dh128_kernel(
    x: jax.Array,
    Wq: jax.Array,
    Wk: jax.Array,
    Wv: jax.Array,
    Wo: jax.Array,
):
    def body(x_hbm, wq_hbm, wk_hbm, wv_hbm, wo_hbm, out_ref,
             x_f32, w_stage, w_bf, x_all, q_s, k_s, v_s, ctx_s,
             cosq_s, sinq_s, cos_s, sin_s,
             send_buf, recv_buf,
             load_sems, ag_send, ag_recv, rs_send, rs_recv):
        my = lax.axis_index("i")

        x_load = pltpu.make_async_copy(x_hbm, x_f32, load_sems.at[0])
        x_load.start()
        w_loads = []
        for j, w in enumerate((wq_hbm, wk_hbm, wv_hbm, wo_hbm)):
            cp = pltpu.make_async_copy(w, w_stage.at[j], load_sems.at[1 + j])
            cp.start()
            w_loads.append(cp)

        x_load.wait()
        x_all[my] = x_f32[...].astype(BF16)

        def ag_copy(k, b):
            return pltpu.make_async_remote_copy(
                src_ref=x_all.at[my, b],
                dst_ref=x_all.at[my, b],
                send_sem=ag_send.at[(k - 1) * 2 + b],
                recv_sem=ag_recv.at[(k - 1) * 2 + b],
                device_id=((my + k) % N_DEV,),
                device_id_type=pl.DeviceIdType.MESH,
            )

        for b in range(B_LOC):
            for k in (1, 3, 2):
                ag_copy(k, b).start()

        lane = lax.broadcasted_iota(jnp.int32, (SQ, DH), 1)
        row = lax.broadcasted_iota(jnp.int32, (SQ, DH), 0).astype(F32)
        pair = (lane // 2).astype(F32)
        inv = jnp.exp(pair * (-2.0 * 9.210340371976184 / DH))
        pos = row * inv
        c = jnp.cos(pos)
        s = jnp.sin(pos)
        even = (lane % 2) == 0
        s_signed = jnp.where(even, -s, s)
        cos_s[...] = c
        sin_s[...] = s_signed
        cosq_s[...] = c * SCALE
        sinq_s[...] = s_signed * SCALE

        for j in range(4):
            w_loads[j].wait()
            w_bf[j] = w_stage[j].astype(BF16)

        def rope(t, c_ref, s_ref):
            sw = jnp.where(even, pltpu.roll(t, DH - 1, 1), pltpu.roll(t, 1, 1))
            return t * c_ref[...] + sw * s_ref[...]

        def compute_ctx(x_src):
            xb = x_src[...]
            for cidx in range(D // CH):
                cs = slice(cidx * CH, (cidx + 1) * CH)
                q = jnp.dot(xb, w_bf[0, :, cs], preferred_element_type=F32)
                kk = jnp.dot(xb, w_bf[1, :, cs], preferred_element_type=F32)
                v = jnp.dot(xb, w_bf[2, :, cs], preferred_element_type=F32)
                for hh in range(CH // DH):
                    hs = slice(hh * DH, (hh + 1) * DH)
                    col = slice(cidx * CH + hh * DH, cidx * CH + (hh + 1) * DH)
                    q_s[:, col] = rope(q[:, hs], cosq_s, sinq_s).astype(BF16)
                    k_s[:, col] = rope(kk[:, hs], cos_s, sin_s).astype(BF16)
                v_s[:, cs] = v.astype(BF16)

            def head(h, carry):
                col = pl.ds(pl.multiple_of(h * DH, DH), DH)
                qh = q_s[:, col]
                kh = k_s[:, col]
                vh = v_s[:, col]
                sc = lax.dot_general(qh, kh, (((1,), (1,)), ((), ())),
                                     preferred_element_type=F32)
                m = jnp.max(sc, axis=-1, keepdims=True)
                p = jnp.exp(sc - m)
                l = jnp.sum(p, axis=-1, keepdims=True)
                o = jnp.dot(p.astype(BF16), vh, preferred_element_type=F32)
                ctx_s[:, col] = (o / l).astype(BF16)
                return carry

            lax.fori_loop(0, HQ, head, 0)

        def rs_copy(k, b):
            return pltpu.make_async_remote_copy(
                src_ref=send_buf.at[k - 1, b],
                dst_ref=recv_buf.at[k - 1, b],
                send_sem=rs_send.at[(k - 1) * 2 + b],
                recv_sem=rs_recv.at[(k - 1) * 2 + b],
                device_id=((my - k) % N_DEV,),
                device_id_type=pl.DeviceIdType.MESH,
            )

        compute_ctx(x_all.at[my, 0])
        out_ref[0] = jnp.dot(ctx_s[...], w_bf[3], preferred_element_type=F32)

        def remote_step(t, carry):
            j = t % 3
            b = t // 3
            k = jnp.where(j == 0, 1, jnp.where(j == 1, 3, 2))
            src = (my - k) % N_DEV
            ag_copy(k, b).wait_recv()
            compute_ctx(x_all.at[src, b])
            send_buf[k - 1, b] = jnp.dot(
                ctx_s[...], w_bf[3], preferred_element_type=F32).astype(BF16)
            rs_copy(k, b).start()
            return carry

        lax.fori_loop(0, 6, remote_step, 0)

        compute_ctx(x_all.at[my, 1])
        out_ref[1] = jnp.dot(ctx_s[...], w_bf[3], preferred_element_type=F32)

        for b in range(B_LOC):
            for k in (1, 2, 3):
                rs_copy(k, b).wait_recv()
            out_ref[b] = (out_ref[b]
                          + recv_buf[0, b].astype(F32)
                          + recv_buf[1, b].astype(F32)
                          + recv_buf[2, b].astype(F32))

        for b in range(B_LOC):
            for k in (1, 2, 3):
                ag_copy(k, b).wait_send()
                rs_copy(k, b).wait_send()

    any_spec = pl.BlockSpec(memory_space=pl.ANY)
    return pl.pallas_call(
        body,
        out_shape=jax.ShapeDtypeStruct((B_LOC, SQ, D), F32),
        in_specs=[any_spec] * 5,
        out_specs=pl.BlockSpec(memory_space=pltpu.VMEM),
        scratch_shapes=[
            pltpu.VMEM((B_LOC, SQ, D), F32),
            pltpu.VMEM((4, D, D), F32),
            pltpu.VMEM((4, D, D), BF16),
            pltpu.VMEM((N_DEV, B_LOC, SQ, D), BF16),
            pltpu.VMEM((SQ, D), BF16),
            pltpu.VMEM((SQ, D), BF16),
            pltpu.VMEM((SQ, D), BF16),
            pltpu.VMEM((SQ, D), BF16),
            pltpu.VMEM((SQ, DH), F32),
            pltpu.VMEM((SQ, DH), F32),
            pltpu.VMEM((SQ, DH), F32),
            pltpu.VMEM((SQ, DH), F32),
            pltpu.VMEM((3, B_LOC, SQ, D), BF16),
            pltpu.VMEM((3, B_LOC, SQ, D), BF16),
            pltpu.SemaphoreType.DMA((5,)),
            pltpu.SemaphoreType.DMA((6,)),
            pltpu.SemaphoreType.DMA((6,)),
            pltpu.SemaphoreType.DMA((6,)),
            pltpu.SemaphoreType.DMA((6,)),
        ],
        compiler_params=pltpu.CompilerParams(
            vmem_limit_bytes=110 * 1024 * 1024,
        ),
    )(x, Wq, Wk, Wv, Wo)
```

```python
import jax
import jax.numpy as jnp
from jax import lax
from jax.experimental import pallas as pl
from jax.experimental.pallas import tpu as pltpu

N_DEV = 4
B_LOC = 2
SQ = 512
D = 1024
HQ = 8
DH = 128
SCALE = 0.08838834764831843 * 1.4426950408889634
CH = 256
NCH = D // CH
N_STEPS = N_DEV * B_LOC

F32 = jnp.float32
BF16 = jnp.bfloat16


def pallas_dist_rope_attn_htp_bs_b2_sq512_d1024_hq8_dh128_kernel(
    x: jax.Array,
    Wq: jax.Array,
    Wk: jax.Array,
    Wv: jax.Array,
    Wo: jax.Array,
):
    def body(x_hbm, wq_hbm, wk_hbm, wv_hbm, wo_hbm, out_buf,
             x_f32, w_stage, w_bf, x_all, q_s, k_s, v_s, ctx_s, res_f32,
             cosq_s, sinq_s, cos_s, sin_s,
             send_buf, recv_buf,
             load_sems, ag_send, ag_recv, rs_send, rs_recv):
        my = lax.axis_index("i")
        w_hbm = (wq_hbm, wk_hbm, wv_hbm, wo_hbm)

        def x_load(b):
            return pltpu.make_async_copy(x_hbm.at[b], x_f32.at[b], load_sems.at[b])

        def w_load(j, cidx):
            rs_ = pl.ds(cidx * CH, CH)
            return pltpu.make_async_copy(w_hbm[j].at[rs_, :], w_stage.at[j, rs_, :],
                                         load_sems.at[2 + j * NCH + cidx])

        def ag_copy(k, b):
            return pltpu.make_async_remote_copy(
                src_ref=x_all.at[my, b],
                dst_ref=x_all.at[my, b],
                send_sem=ag_send.at[(k - 1) * 2 + b],
                recv_sem=ag_recv.at[(k - 1) * 2 + b],
                device_id=((my + k) % N_DEV,),
                device_id_type=pl.DeviceIdType.MESH,
            )

        def rs_copy(k, b):
            return pltpu.make_async_remote_copy(
                src_ref=send_buf.at[(k - 1) * 2 + b],
                dst_ref=recv_buf.at[k - 1, b],
                send_sem=rs_send.at[(k - 1) * 2 + b],
                recv_sem=rs_recv.at[(k - 1) * 2 + b],
                device_id=((my - k) % N_DEV,),
                device_id_type=pl.DeviceIdType.MESH,
            )

        x_load(0).start()
        for cidx in range(NCH):
            w_load(0, cidx).start()

        x_load(0).wait()
        x_all[my, 0] = x_f32[0].astype(BF16)
        for k in (1, 3):
            ag_copy(k, 0).start()
        for j in (1, 2):
            for cidx in range(NCH):
                w_load(j, cidx).start()

        lane = lax.broadcasted_iota(jnp.int32, (SQ, DH), 1)
        row = lax.broadcasted_iota(jnp.int32, (SQ, DH), 0).astype(F32)
        pair = (lane // 2).astype(F32)
        inv = jnp.exp(pair * (-2.0 * 9.210340371976184 / DH))
        pos = row * inv
        c = jnp.cos(pos)
        s = jnp.sin(pos)
        s_signed = jnp.where((lane % 2) == 0, -s, s)
        cos_s[...] = c
        sin_s[...] = s_signed
        cosq_s[...] = c * SCALE
        sinq_s[...] = s_signed * SCALE

        def rope(t, c_ref, s_ref):
            even = (lax.broadcasted_iota(jnp.int32, (SQ, DH), 1) % 2) == 0
            sw = jnp.where(even, pltpu.roll(t, DH - 1, 1), pltpu.roll(t, 1, 1))
            return t * c_ref[...] + sw * s_ref[...]

        def step(t, carry):
            b = t // N_DEV
            r = t % N_DEV
            rr = jnp.where(b == 0, r, (r + 1) % N_DEV)
            k = jnp.where(rr == 2, 3, jnp.where(rr == 3, 2, rr))
            src = (my - k) % N_DEV
            first = t == 0

            @pl.when(k > 0)
            def _():
                ag_copy(k, b).wait_recv()

            x_src = x_all.at[src, b]

            xb = x_src[...]
            for j in range(3):
                @pl.when(first)
                def _():
                    for cidx in range(NCH):
                        w_load(j, cidx).wait()
                    if j == 1:
                        x_load(1).start()
                        for cidx in range(NCH):
                            w_load(3, cidx).start()
                    w_bf[j] = w_stage[j].astype(BF16)

                for cidx in range(NCH):
                    cs = slice(cidx * CH, (cidx + 1) * CH)
                    tt = jnp.dot(xb, w_bf[j, :, cs], preferred_element_type=F32)
                    if j == 2:
                        v_s[:, cs] = tt.astype(BF16)
                    else:
                        dst = q_s if j == 0 else k_s
                        c_ref, s_ref = (cosq_s, sinq_s) if j == 0 else (cos_s, sin_s)
                        for hh in range(CH // DH):
                            col = slice(cidx * CH + hh * DH, cidx * CH + (hh + 1) * DH)
                            dst[:, col] = rope(tt[:, hh * DH:(hh + 1) * DH],
                                               c_ref, s_ref).astype(BF16)

            def head(h, c2):
                col = pl.ds(pl.multiple_of(h * DH, DH), DH)
                qh = q_s[:, col]
                kh = k_s[:, col]
                vh = v_s[:, col]
                sc = lax.dot_general(qh, kh, (((1,), (1,)), ((), ())),
                                     preferred_element_type=F32)
                m = jnp.max(sc, axis=-1, keepdims=True)
                p = jnp.exp2(sc - m)
                l = jnp.sum(p, axis=-1, keepdims=True)
                o = jnp.dot(p.astype(BF16), vh, preferred_element_type=F32)
                ctx_s[:, col] = (o / l).astype(BF16)
                return c2

            lax.fori_loop(0, HQ, head, 0, unroll=8)

            @pl.when(first)
            def _():
                ag_copy(2, 0).start()
                x_load(1).wait()
                x_all[my, 1] = x_f32[1].astype(BF16)
                for cidx in range(NCH):
                    w_load(3, cidx).wait()
                w_bf[3] = w_stage[3].astype(BF16)

            f32_slot = jnp.where(k == 0, b, B_LOC)
            bf_slot = jnp.where(k == 0, 6, (k - 1) * 2 + b)
            res = jnp.dot(ctx_s[...], w_bf[3], preferred_element_type=F32)
            res_f32[f32_slot] = res
            send_buf[bf_slot] = res.astype(BF16)

            @pl.when(k > 0)
            def _():
                rs_copy(k, b).start()

            @pl.when(first)
            def _():
                ag_copy(1, 1).start()
                ag_copy(3, 1).start()

            @pl.when(t == 1)
            def _():
                ag_copy(2, 1).start()

            return carry

        lax.fori_loop(0, N_STEPS, step, 0)

        for b in range(B_LOC):
            for k in (1, 2, 3):
                rs_copy(k, b).wait_recv()
            out_buf[b] = (res_f32[b]
                          + recv_buf[0, b].astype(F32)
                          + recv_buf[1, b].astype(F32)
                          + recv_buf[2, b].astype(F32))

        for b in range(B_LOC):
            for k in (1, 2, 3):
                ag_copy(k, b).wait_send()
                rs_copy(k, b).wait_send()

    hbm_spec = pl.BlockSpec(memory_space=pltpu.MemorySpace.HBM)
    return pl.pallas_call(
        body,
        out_shape=jax.ShapeDtypeStruct((B_LOC, SQ, D), F32),
        in_specs=[hbm_spec] * 5,
        out_specs=pl.BlockSpec(memory_space=pltpu.VMEM),
        scratch_shapes=[
            pltpu.VMEM((B_LOC, SQ, D), F32),
            pltpu.VMEM((4, D, D), F32),
            pltpu.VMEM((4, D, D), BF16),
            pltpu.VMEM((N_DEV, B_LOC, SQ, D), BF16),
            pltpu.VMEM((SQ, D), BF16),
            pltpu.VMEM((SQ, D), BF16),
            pltpu.VMEM((SQ, D), BF16),
            pltpu.VMEM((SQ, D), BF16),
            pltpu.VMEM((B_LOC + 1, SQ, D), F32),
            pltpu.VMEM((SQ, DH), F32),
            pltpu.VMEM((SQ, DH), F32),
            pltpu.VMEM((SQ, DH), F32),
            pltpu.VMEM((SQ, DH), F32),
            pltpu.VMEM((7, SQ, D), BF16),
            pltpu.VMEM((3, B_LOC, SQ, D), BF16),
            pltpu.SemaphoreType.DMA((2 + 4 * NCH,)),
            pltpu.SemaphoreType.DMA((6,)),
            pltpu.SemaphoreType.DMA((6,)),
            pltpu.SemaphoreType.DMA((6,)),
            pltpu.SemaphoreType.DMA((6,)),
        ],
        compiler_params=pltpu.CompilerParams(
            vmem_limit_bytes=110 * 1024 * 1024,
        ),
    )(x, Wq, Wk, Wv, Wo)
```
